```python
import numpy as np

kernel_name = "dist_moe_cap_ep_tokshard_n2048_d512_e8_h1024"

def setup_inputs():
    x = np.random.randn(8192, 512).astype(np.float32)
    router_W = np.random.randn(512, 32).astype(np.float32) * 0.1
    scores64 = x.astype(np.float64) @ router_W.astype(np.float64)
    route_idx = np.argsort(-scores64, axis=-1)[:, :1].astype(np.int32)
    expert_W = np.random.randn(32, 512, 1024).astype(np.float32) * 0.02
    return {"x": x, "router_W": router_W, "route_idx": route_idx, "expert_W": expert_W}

def reference(x, router_W, route_idx, expert_W):
    counts = np.zeros(32, dtype=np.int64)
    out = np.zeros((8192, 1024), dtype=np.float32)
    for i in range(8192):
        e = int(route_idx[i, 0])
        if counts[e] < 204:
            out[i] = x[i] @ expert_W[e]
            counts[e] += 1
    return out
```

```python
import functools

import jax
import jax.numpy as jnp
from jax import lax
from jax.experimental import pallas as pl
from jax.experimental.pallas import tpu as pltpu

NDEV = 4
T = 2048
D = 512
H = 1024
E = 32
EL = 8
CAP = 204
CAPM = 208
MS = 96
CAPF = 256
LANES = 128

XR = 2
YR = 3
CHD = 16
GD = CHD // XR
GM = 16
SQ = 26
NSQ = EL * CAP // GM + 1
GC = 8
CH = GC * YR
PR = 8
PCAP = EL * CAP + 2 * PR
LA = 128
LCAP = LA + 13 * LA
FS = CAPM

XB = 32
YB = 16

NXC = 8
XC = T // NXC
WAVES = ((1, 0, 4), (1, 4, 8), (3, 0, 2), (5, 0, 1))
FLUSH = len(WAVES) - 1
WC = tuple(sorted({w[0] for w in WAVES}))
NW = len(WC)
KLATE = max(w[2] for w in WAVES if w[0] != WC[0])

SD = NSQ * GM + WC[0] * XC + KLATE * CAP + 2 * XB + GM
SD = (SD + GD - 1) // GD * GD
DB = 16
SC = EL * CAP + YB + GC + DB
SC = (SC + GC - 1) // GC * GC

FL = 2
DMIN = 29
XSCALE = 880
BIAS = {(1, 0): 4, (2, 1): -7, (3, 2): -7, (1, 2): -4, (2, 3): -3}

U32 = jnp.uint32
_scope = jax.named_scope
MESH = pl.DeviceIdType.MESH


def _div_pow2(a, g):
    return a >> (g.bit_length() - 1)


def _cdiv_pow2(a, g):
    return _div_pow2(a + (g - 1), g)


def _pack(lo, hi):
    lo = lax.bitcast_convert_type(lo, U32) + U32(0x8000)
    hi = lax.bitcast_convert_type(hi, U32) + U32(0x8000)
    return (lo >> 16) | (hi & U32(0xFFFF0000))


def _unpack_lo(w):
    return lax.bitcast_convert_type(w << 16, jnp.float32)


def _unpack_hi(w):
    return lax.bitcast_convert_type(w & U32(0xFFFF0000), jnp.float32)


def _move(x, src_bit, dst_bit):
    if src_bit >= dst_bit:
        return x >> (src_bit - dst_bit) if src_bit > dst_bit else x
    return x << (dst_bit - src_bit)


def _encode(w, n, eref, planes):
    d = eref - (w & U32(0x7F807F80))
    nib = U32(0x000F000F << (4 * n))
    byte = (w & U32(0x007F007F)) | ((w >> 8) & U32(0x00800080))
    parts = ((n // 2, byte << 8 if n % 2 else byte),
             (2, _move(d, 7, 4 * n) & nib),
             (3, _move(d, 11, 4 * n) & nib))
    for i, v in parts:
        planes[i] = v if planes[i] is None else planes[i] | v


def _decode(planes, n, eref):
    b = planes[n // 2] >> 8 if n % 2 else planes[n // 2]
    d = _move(planes[2], 4 * n, 7) & U32(0x07800780)
    if planes[3] is not None:
        d = d | (_move(planes[3], 4 * n, 11) & U32(0x78007800))
    return (((b << 8) & U32(0x80008000)) | ((eref - d) & U32(0x7F807F80))
            | (b & U32(0x007F007F)))


def _nonzero_rows(need, bounds):
    r = need.shape[0]
    bf = jnp.bfloat16
    g = jnp.broadcast_to(
        jnp.max(jnp.where(need, 1.0, 0.0), axis=1, keepdims=True), (r, LANES))
    tri = (lax.broadcasted_iota(jnp.int32, (r, r), 1)
           < lax.broadcasted_iota(jnp.int32, (r, r), 0))
    pre = jnp.dot(jnp.where(tri, 1.0, 0.0).astype(bf), g.astype(bf),
                  preferred_element_type=jnp.float32)
    lane = lax.broadcasted_iota(jnp.int32, (r, LANES), 1).astype(jnp.float32)
    hot = jnp.concatenate(
        [jnp.where(pre == lane, g, 0.0),
         jnp.where((pre == lane + LANES) | (lane == LANES - 1), g, 0.0)], axis=1)
    col = lax.broadcasted_iota(jnp.int32, (8, r), 1)
    sel = lax.broadcasted_iota(jnp.int32, (8, r), 0)
    wts = jnp.where(sel == 0, col, 0)
    for i, bnd in enumerate(bounds):
        wts = jnp.where((sel == i + 1) & (col < bnd), 1, wts)
    return jnp.dot(wts.astype(jnp.float32).astype(bf), hot.astype(bf),
                   preferred_element_type=jnp.float32).astype(jnp.int32)


def _wait_chunks(buf, sem, n, nmax, ch=CH):
    def one(v):
        pltpu.make_async_copy(buf.at[pl.ds(0, v * ch)], buf.at[pl.ds(0, v * ch)],
                              sem).wait()

    def tree(lo, hi):
        if lo == hi:
            if lo:
                one(lo)
            return
        mid = (lo + hi) // 2
        lax.cond(n <= mid, lambda: tree(lo, mid), lambda: tree(mid + 1, hi))

    tree(0, nmax)


def _copy_fwd(src, srow, dst, drow, ntok, rows_per_tok, blk_tok):
    br = blk_tok * rows_per_tok

    def body(i, c):
        dst[pl.ds(drow + i * br, br), :] = src[pl.ds(srow + i * br, br), :]
        return c

    lax.fori_loop(0, _cdiv_pow2(ntok, blk_tok), body, 0)


def _copy_bwd(src, srow, dst, drow, ntok, rows_per_tok, blk_tok):
    br = blk_tok * rows_per_tok
    end = ntok * rows_per_tok

    def body(i, c):
        o = end - (i + 1) * br
        dst[pl.ds(drow + o, br), :] = src[pl.ds(srow + o, br), :]
        return c

    lax.fori_loop(0, _cdiv_pow2(ntok, blk_tok), body, 0)


def _prefix(vals, start):
    out = [start]
    for v in vals:
        out.append(out[-1] + v)
    return out


def _batches(off, g, sent):
    lo, hi, first = [], [], []
    grp = jnp.int32(0)
    for k in range(EL):
        rnd = _cdiv_pow2 if k == EL - 1 else _div_pow2
        h = rnd(off[k + 1], g)
        f = jnp.where(sent * g >= off[k], k, grp)
        lo.append(sent)
        hi.append(h)
        first.append(f)
        grp = jnp.where(h > sent, k, f)
        sent = h
    return lo, hi, first


def _kernel(x_hbm, idx_hbm, w_hbm, out_ref,
            xv, wv, idx_v, pos_v, hist_v, xt, sbf, sb, rs, eb, rb, css, csr, fb,
            pb, pss, psr, er_out, er_in, flag_v, lb, st, sq, rq, ctl_v, tmp,
            pos_s, inv_s, hist_s, nacc_s, flag_s, lst_out, lst_in, tab_s, ctl_s,
            xsem, wsem, msem, hsem, dsem, csem, fsem, ssem,
            esem, gsem, lsem, psem, qsem, ksem):
    me = lax.axis_index("i")
    rem = range(1, NDEV)

    def chip(j):
        return (me + j) & (NDEV - 1)

    idx_cp = pltpu.make_async_copy(idx_hbm, idx_v, msem.at[0])
    idx_cp.start()
    x_cps = [pltpu.make_async_copy(x_hbm.at[pl.ds(c * XC, XC)],
                                   xv.at[pl.ds(c * XC, XC)], xsem.at[c])
             for c in range(NXC)]
    x_cps[0].start()
    bar = pltpu.get_barrier_semaphore()
    for j in rem:
        pl.semaphore_signal(bar, inc=1, device_id=(chip(j),), device_id_type=MESH)
    idx_cp.wait()
    for cp in x_cps[1:]:
        cp.start()
    w_cps = [pltpu.make_async_copy(w_hbm.at[k], wv.at[k], wsem.at[k])
             for k in range(EL)]
    for cp in w_cps:
        cp.start(priority=1)

    def hist_slot(q):
        return hist_s.at[pl.ds(pl.multiple_of(q * LANES, LANES), LANES)]

    with _scope("s_route"):
        idx = idx_v[...]
        nb = T // LANES
        eio = lax.broadcasted_iota(jnp.int32, (E, LANES), 0)
        ohs = [jnp.broadcast_to(idx[b:b + 1, :], (E, LANES)) == eio
               for b in range(nb)]
        ohf = [jnp.where(o, 1.0, 0.0) for o in ohs]

        osum = ohf[0]
        part = []
        for b in range(1, nb):
            if b * LANES in [c * XC for c in WC]:
                part.append(osum)
            osum = osum + ohf[b]
        pads = [jnp.zeros((LANES - (NW + 1) * E, LANES), jnp.float32)] if NW < 3 else []
        osum = jnp.concatenate([osum] + part + pads, axis=0)
        hist = lax.dot_general(jnp.ones((8, LANES), jnp.bfloat16),
                               osum.astype(jnp.bfloat16),
                               (((1,), (1,)), ((), ())),
                               preferred_element_type=jnp.float32)
        hist_v[...] = hist.astype(jnp.int32)
        pltpu.make_async_copy(hist_v.at[0], hist_slot(me), hsem.at[me]).start()

    with _scope("s_rank"):
        oh = jnp.concatenate(ohf, axis=0).astype(jnp.bfloat16)
        ur = lax.broadcasted_iota(jnp.int32, (LANES, 2 * LANES), 0)
        uc = lax.broadcasted_iota(jnp.int32, (LANES, 2 * LANES), 1)
        tri = jnp.where((ur < uc) | (uc >= LANES), 1.0, 0.0).astype(jnp.bfloat16)
        pre = jnp.dot(oh, tri, preferred_element_type=jnp.float32)
        carry = jnp.zeros((E, LANES), jnp.float32)
        rows = []
        for b in range(nb):
            before = pre[b * E:(b + 1) * E, 0:LANES] + carry
            rows.append(jnp.sum(jnp.where(ohs[b], before, 0.0), axis=0,
                                keepdims=True))
            carry = carry + pre[b * E:(b + 1) * E, LANES:2 * LANES]
        rank = jnp.concatenate(rows, axis=0).astype(jnp.int32)
        pos_v[...] = (idx * CAPF + jnp.minimum(rank, CAPF - 1) + XB) * XR
        pos_cp = pltpu.make_async_copy(pos_v, pos_s, msem.at[1])
        pos_cp.start()

    def hist_wait(q):
        pltpu.make_async_copy(hist_v.at[0], hist_slot(q), hsem.at[q]).wait()

    def seen(s, d, k, w):
        return jnp.minimum(hist_s[s * LANES + (w + 1) * E + d * EL + k], CAP)

    def send_chunk(src, srow, dst, drow, rsem, dv, ch):
        pltpu.make_async_remote_copy(
            src_ref=src.at[pl.ds(pl.multiple_of(srow, 2), ch)],
            dst_ref=dst.at[pl.ds(pl.multiple_of(drow, 2), ch)],
            send_sem=ssem.at[0 if src is sb else 2 if src is pss else 4],
            recv_sem=rsem,
            device_id=(dv,),
            device_id_type=MESH).start()

    def send_res(src, stok, dst, dtok, rsem, dv):
        pltpu.make_async_remote_copy(
            src_ref=src.at[:, pl.ds(pl.multiple_of(stok, GC), GC)],
            dst_ref=dst.at[:, pl.ds(pl.multiple_of(dtok, GC), GC)],
            send_sem=ssem.at[1], recv_sem=rsem, device_id=(dv,),
            device_id_type=MESH).start()

    def send_ranges(lo, hi, send_one):
        cnt = {j: hi[j] - lo[j] for j in rem}
        m = jnp.maximum(jnp.maximum(cnt[1], cnt[2]), cnt[3])

        def body(i, c):
            for j in rem:
                pl.when(i < cnt[j])(lambda j=j: send_one(j, lo[j] + i))
            return c

        lax.fori_loop(0, m, body, 0)
        return cnt[1] + cnt[2] + cnt[3]

    def send_x(j, c, grp):
        send_chunk(sb, (j - 1) * SD * XR + c * CHD,
                   rs, ((NDEV - j - 1) * SD + XB) * XR + c * CHD,
                   dsem.at[grp], chip(j), CHD)

    def compact(j, k, r0, n, pos, blk):
        _copy_fwd(sbf, ((chip(j) * EL + k) * CAPF + XB + r0) * XR,
                  sb, ((j - 1) * SD + pos) * XR, n, XR, blk)

    nsent = jnp.int32(0)
    wpos = {j: jnp.int32(0) for j in rem}
    wsent = {j: jnp.int32(0) for j in rem}
    done = {j: [jnp.int32(0)] * EL for j in rem}
    for c in range(NXC):
        with _scope("s_xwait"):
            x_cps[c].wait()

        def pack_body(i, carry_, c=c):
            r = pl.multiple_of(c * XC + i * 8, 8)
            v = xv[pl.ds(r, 8), :]
            w = _pack(v[:, 0:D // 2], v[:, D // 2:D])
            xt[pl.ds(r * XR, 8, stride=XR), :] = w[:, 0:LANES]
            xt[pl.ds(r * XR + 1, 8, stride=XR), :] = w[:, LANES:2 * LANES]
            return carry_

        with _scope("s_pack"):
            lax.fori_loop(0, XC // 8, pack_body, 0, unroll=4)
            if c == 1:
                xtop = lax.bitcast_convert_type(xv[0:64, :], jnp.int32) & 0x7F800000
                xtop = jnp.max(jnp.max(xtop, axis=0, keepdims=True), axis=1,
                               keepdims=True)
                xtop = jnp.minimum((xtop >> 16) + (3 << 7), 0x7F80) | 0x8000
                xref = lax.bitcast_convert_type(jnp.broadcast_to(
                    xtop | (xtop << 16), (1, LANES)), U32)
            if c:
                r0 = (0 if c == 1 else c) * XC * XR
                d = xref - (xt[r0:(c + 1) * XC * XR, :] & U32(0x7F807F80))
                while d.shape[0] > 8:
                    d = d[0:d.shape[0] // 2] | d[d.shape[0] // 2:]
                span = d if c == 1 else span | d
        if c == 0:
            pos_cp.wait()

        def scat_body(i, carry_, c=c):
            b = c * (XC // LANES) + i
            for u in range(LANES):
                sbf[pl.ds(pos_s[b, u], XR), :] = xt[pl.ds((b * LANES + u) * XR, XR), :]
            return carry_

        with _scope("s_scat"):
            lax.fori_loop(0, XC // LANES, scat_body, 0)

        if c + 1 not in WC:
            continue
        w = WC.index(c + 1)
        if w == 0:
            hist_wait(me)
        if w == 1:
            with _scope("s_histwait"):
                for m in range(NDEV):
                    @pl.when(me == m)
                    def _(m=m):
                        for q in range(m):
                            hist_wait(q)
                        for e in range(E):
                            room = jnp.int32(CAP)
                            for q in range(m):
                                room = room - hist_s[q * LANES + e]
                            nacc_s[m * E + e] = jnp.clip(
                                room, 0, hist_s[m * LANES + e])
            nacc_me = [[nacc_s[me * E + chip(j) * EL + k] for k in range(EL)]
                       for j in range(NDEV)]
            for j in rem:
                for k in range(EL):
                    done[j][k] = jnp.minimum(done[j][k], nacc_me[j][k])
        for i, (wc, k0, k1) in enumerate(WAVES):
            if wc != c + 1:
                continue
            with _scope("s_wave"):
                for k in range(k0, k1):
                    for j in rem:
                        r = seen(me, chip(j), k, w)
                        if w:
                            r = jnp.minimum(r, nacc_me[j][k])
                        compact(j, k, done[j][k], r - done[j][k], wpos[j], 16)
                        wpos[j] = wpos[j] + (r - done[j][k])
                        done[j][k] = r
            if i == 0:
                with _scope("s_barrier"):
                    pl.semaphore_wait(bar, NDEV - 1)
                for j in rem:
                    pltpu.make_async_remote_copy(
                        src_ref=hist_v.at[0], dst_ref=hist_slot(me),
                        send_sem=msem.at[2], recv_sem=hsem.at[me],
                        device_id=(chip(j),), device_id_type=MESH).start()
            with _scope("s_wsend"):
                rnd = _cdiv_pow2 if i == FLUSH else _div_pow2
                hi = {j: rnd(wpos[j], GD) for j in rem}
                nsent = nsent + send_ranges(
                    wsent, hi,
                    lambda j, ch, i=i: send_x(j, ch, EL if i <= FLUSH else 0))
                wsent = hi
                if i == FLUSH:
                    wpos = {j: hi[j] * GD for j in rem}

    def ctl_slot(q):
        return ctl_s.at[pl.ds(pl.multiple_of(q * LANES, LANES), LANES)]

    with _scope("s_dispatch"):
        wide = lax.bitcast_convert_type(span & U32(0x70007000), jnp.int32)
        wide = jnp.max(jnp.max(wide, axis=0, keepdims=True), axis=1, keepdims=True)
        lane0 = lax.broadcasted_iota(jnp.int32, (1, LANES), 1) == 0
        ctl_v[0:1, :] = jnp.where(lane0, wide,
                                  lax.bitcast_convert_type(xref, jnp.int32))
        ctl_cp = pltpu.make_async_copy(ctl_v.at[0], ctl_slot(0), ksem.at[0])
        ctl_cp.start()
        for j in rem:
            pltpu.make_async_remote_copy(
                src_ref=ctl_v.at[0], dst_ref=ctl_slot(NDEV - j),
                send_sem=msem.at[2], recv_sem=ksem.at[NDEV - j],
                device_id=(chip(j),), device_id_type=MESH).start()
        offm = {j: _prefix([nacc_me[j][k] - done[j][k] for k in range(EL)],
                           jnp.int32(0)) for j in rem}
        xbat = {j: _batches(offm[j], GM, jnp.int32(0)) for j in rem}

        def squeeze_chunk(j, c, carry_):
            row = ((j - 1) * SD + wpos[j] + c * GM) * XR
            planes = [None] * 4
            for n in range(XR):
                _encode(sb[pl.ds(row + n, GM, stride=XR), :], n, xref, planes)
            top = (planes[3][0:8] | (planes[3][8:16] << 8)) & U32(0x11111111)
            dst = ((j - 1) * NSQ + c) * SQ
            sq[pl.ds(dst, GM), :] = planes[0]
            sq[pl.ds(dst + GM, 8), :] = planes[2][0:8] | (planes[2][8:16] << 8)
            sq[pl.ds(dst + GM + 8, 2), :] = functools.reduce(
                jnp.bitwise_or, [top[2 * i:2 * i + 2] << i for i in range(4)])
            return carry_

        def send_sq(j, c, grp):
            send_chunk(sq, ((j - 1) * NSQ + c) * SQ,
                       rq, ((NDEV - j - 1) * NSQ + c) * SQ,
                       qsem.at[grp], chip(j), SQ)

        def send_raw(j, c, grp):
            send_chunk(sb, ((j - 1) * SD + wpos[j] + c * GM) * XR,
                       rs, ((NDEV - j - 1) * SD + XB + wpos[j] + c * GM) * XR,
                       dsem.at[grp], chip(j), GM * XR)

        for k in range(EL):
            for j in rem:
                compact(j, k, done[j][k], nacc_me[j][k] - done[j][k],
                        wpos[j] + offm[j][k], XB)
            if k == 0:
                ctl_cp.wait()
                squeeze = ctl_s[0] == 0
            if k == EL - 1:
                for j in rem:
                    sb[pl.ds(((j - 1) * SD + wpos[j] + offm[j][EL]) * XR, GM * XR),
                       :] = jnp.zeros((GM * XR, LANES), U32)
            lo = {j: xbat[j][0][k] for j in rem}
            hi = {j: xbat[j][1][k] for j in rem}

            def grouped(send, k=k):
                return lambda j, ch: send(
                    j, ch, jnp.where(ch == xbat[j][0][k], xbat[j][2][k], k))

            @pl.when(squeeze)
            def _(lo=lo, hi=hi, grouped=grouped):
                def three(i, c_):
                    for j in rem:
                        squeeze_chunk(j, jnp.minimum(lo[j] + i, NSQ - 1), c_)
                    return c_

                lax.fori_loop(
                    0, functools.reduce(jnp.maximum, [hi[j] - lo[j] for j in rem]),
                    three, 0)
                send_ranges(lo, hi, grouped(send_sq))

            @pl.when(jnp.logical_not(squeeze))
            def _(lo=lo, hi=hi, grouped=grouped):
                send_ranges(lo, hi, grouped(send_raw))

        nmain = sum(xbat[j][1][EL - 1] for j in rem)
        nsent = nsent + jnp.where(squeeze, 0, nmain * (GM // GD))
        nsq = jnp.where(squeeze, nmain, 0)

    with _scope("s_prep"):
        for q in rem:
            pl.when(q > me)(lambda q=q: hist_wait(q))
        ntot = [[jnp.int32(0)] * NDEV for _ in range(NDEV)]
        for e in range(E):
            room = jnp.int32(CAP)
            for s in range(NDEV):
                h = hist_s[s * LANES + e]
                a = jnp.clip(room, 0, h)
                nacc_s[s * E + e] = a
                ntot[s][e // EL] = ntot[s][e // EL] + a
                room = room - h

        nacc_in = [nacc_me[0]] + [
            [nacc_s[chip(q) * E + me * EL + k] for k in range(EL)] for q in rem]
        pieces = {q: [[] for _ in range(EL)] for q in rem}
        offin, early, nflush = {}, {}, {}
        for q in rem:
            pos = jnp.int32(0)
            dn = [jnp.int32(0)] * EL
            for i, (wc, k0, k1) in enumerate(WAVES):
                w = WC.index(wc)
                for k in range(k0, k1):
                    full = seen(chip(q), me, k, w)
                    r = jnp.minimum(full, nacc_in[q][k])
                    pieces[q][k].append((dn[k], r - dn[k], pos))
                    pos = pos + ((r - dn[k]) if w else full)
                    dn[k] = r
                if i == FLUSH:
                    nflush[q] = _cdiv_pow2(pos, GD)
                    pos = nflush[q] * GD
                    early[q] = dn[0]
                    nearly = len(pieces[q][0])
            offin[q] = _prefix([nacc_in[q][k] - dn[k] for k in range(EL)],
                               jnp.int32(0))
            for k in range(EL):
                pieces[q][k].append(
                    (dn[k], nacc_in[q][k] - dn[k], pos + offin[q][k]))
        offc_out = {q: _prefix(nacc_in[q], jnp.int32(0)) for q in rem}
        bat = {q: _batches(offc_out[q], GC, _div_pow2(early[q], GC)) for q in rem}

        cc = [[_cdiv_pow2(ntot[b][a], GC) for b in range(NDEV)] for a in range(NDEV)]
        cd = [[(ntot[a][b] * (XSCALE * XR // CH)) >> 10 for b in range(NDEV)]
              for a in range(NDEV)]
        load = {}
        for a in range(NDEV):
            h, c = a ^ 3, a ^ 2
            load[(a, h)] = (jnp.maximum(cd[a][h] + cd[a][c], DMIN)
                            + cc[a][h] + cc[a][c] + BIAS.get((a, h), 0))
            used = jnp.minimum(
                DMIN, cd[h][c] + jnp.minimum(cd[a][c], DMIN // 2))
            load[(h, c)] = (cd[h][c] + cd[a][c] + cc[h][c] + cc[a][c]
                            + (DMIN + BIAS.get((h, c), 0)) - used)
        moved = [jnp.int32(0)] * NDEV
        for a in (2, 3, 2, 3, 0, 1, 2, 3):
            h, c, r = a ^ 3, a ^ 2, a ^ 1
            top = jnp.maximum(load[(a, h)], load[(h, c)])
            gap = top - jnp.maximum(load[(a, r)], load[(r, c)])
            mv = jnp.clip(gap >> 1, 0, cc[a][c] - moved[a])
            worst = functools.reduce(jnp.maximum, load.values())
            mv = jnp.where((top + 64 // CH >= worst) & (moved[a ^ 3] == 0), mv, 0)
            moved[a] = moved[a] + mv
            for lk in ((a, h), (h, c)):
                load[lk] = load[lk] - mv
            for lk in ((a, r), (r, c)):
                load[lk] = load[lk] + mv
        rel_out = jnp.int32(0)
        rel_in = jnp.int32(0)
        for a in range(NDEV):
            first = cc[a][a ^ 2] - moved[a]
            rel_out = jnp.where(me == a, first, rel_out)
            rel_in = jnp.where(me == (a ^ 1), first, rel_in)
        foff = _prefix(
            [nacc_s[(me ^ 3) * E + (me ^ 1) * EL + k] for k in range(EL)],
            jnp.int32(0))
        fbat = _batches(foff, GC, jnp.int32(0))

    alink = ((wpos[2] + offm[2][EL] + jnp.where(
        (me & 1) == 1, wpos[1] + offm[1][EL], wpos[3] + offm[3][EL]))
        * (XSCALE * XR // CH)) >> 10

    def group_of(c, off):
        g = jnp.int32(0)
        for k in range(1, EL):
            g = g + jnp.where(c * GC >= off[k], 1, 0)
        return g

    def send_y(q, c, grp):
        send_res(css, (q - 1) * SC + c * GC, csr, (NDEV - q - 1) * SC + DB + c * GC,
                 csem.at[(NDEV - q - 1) * EL + grp], chip(q))

    def send_diag(c):
        send_y(2, c, group_of(c, offc_out[2]))

    def send_diag_range(lo, hi):
        def body(c, carry_):
            send_diag(c)
            return carry_

        lax.fori_loop(lo, hi, body, 0)

    def forward(k, held):
        lo = tab_s[48 + k]
        hi = tab_s[49 + k]
        _wait_chunks(xt, fsem.at[k], hi - lo, (CAP + GC - 1) // GC + 1)

        def body(c, h):
            send_res(fb, c * GC, csr, SC + DB + c * GC,
                     csem.at[EL + group_of(c, foff)], me ^ 3)
            pl.when(h < rel_out)(lambda: send_diag(h))
            return h + 1

        return lax.fori_loop(lo, hi, body, held)

    npat = {q: jnp.int32(0) for q in rem}
    finds, scans = [], []

    def scan(flag_cp, step, k, lo_k, rank0):
        flag_cp.wait()
        lo = jnp.int32(0)
        for q in rem:
            hi = flag_s[step * 8 + q, 2 * LANES - 1]
            code0 = k * CAPF + rank0[q] - lo_k[q]
            dst = npat[q] - lo

            def body(i, c, q=q, code0=code0, dst=dst):
                r = flag_s[step * 8, i]
                pss[pl.ds((q - 1) * PCAP + dst + i, 1), :] = pb[pl.ds(step * FS + r, 1), :]
                lst_out[(q - 1) * LCAP + 2 + dst + i] = (code0 + r) * XR
                return c

            lax.fori_loop(lo, hi, body, 0)
            npat[q] = dst + hi
            lo = hi

    def list_copy(q, lo, n, sem):
        return pltpu.make_async_remote_copy(
            src_ref=lst_out.at[pl.ds((q - 1) * LCAP + lo, n)],
            dst_ref=lst_in.at[pl.ds((NDEV - q - 1) * LCAP + lo, n)],
            send_sem=lsem.at[6 + sem * 3 + q - 1],
            recv_sem=lsem.at[sem * 3 + NDEV - q - 1],
            device_id=(chip(q),), device_id_type=MESH)

    def send_patches(npat1):
        for q in rem:
            lst_out[(q - 1) * LCAP] = npat[q]
            lst_out[(q - 1) * LCAP + 1] = npat1[q]
            list_copy(q, 0, LA, 0).start()
            pl.when(npat[q] > LA - 2)(
                lambda q=q: list_copy(q, LA, LCAP - LA, 1).start())
            nch = _cdiv_pow2(npat[q], PR)

            def body(c, carry_, q=q, nch=nch):
                sem = (NDEV - q - 1) * 2 + jnp.where(c < (nch >> 4) << 4, 0, 1)
                send_chunk(pss, (q - 1) * PCAP + c * PR,
                           psr, (NDEV - q - 1) * PCAP + c * PR,
                           psem.at[sem], chip(q), PR)
                return carry_

            lax.fori_loop(0, nch, body, 0)

    def unsqueeze(q, c, carry_):
        src = ((q - 1) * NSQ + c) * SQ
        ref = lax.bitcast_convert_type(
            jnp.full((1, LANES), ctl_s[q * LANES + 1], jnp.int32), U32)
        low = rq[pl.ds(src + GM, 8), :]
        top = rq[pl.ds(src + GM + 8, 2), :]
        top = jnp.concatenate([top >> i for i in range(4)], axis=0) & U32(0x11111111)
        planes = [rq[pl.ds(src, GM), :], None,
                  jnp.concatenate([low, low >> 8], axis=0),
                  jnp.concatenate([top, top >> 8], axis=0)]
        row = ((q - 1) * SD + XB + nflush[q] * GD + c * GM) * XR
        for n in range(XR):
            tmp[pl.ds(n, GM, stride=XR), :] = _decode(planes, n, ref)
        rs[pl.ds(row, GM * XR), :] = tmp[...]
        return carry_

    dsent = jnp.int32(0)
    for step in range(EL + 1):
        k = max(step - 1, 0)
        zero = jnp.int32(0)
        if step == 0:
            parts = {q: pieces[q][0][:nearly] for q in rem}
            cnt = [nacc_in[0][0]] + [early[q] for q in rem]
            rank0 = {q: zero for q in rem}
            n_in = sum(nflush[q] for q in rem)
            nmax = (KLATE * CAP + 3 * WC[0] * XC + 3 * (GD - 1)) // GD
            lo = {q: zero for q in rem}
            hi = {q: bat[q][0][0] for q in rem}
            first = {q: zero for q in rem}
        else:
            if step == 1:
                parts = {q: pieces[q][0][nearly:] for q in rem}
                cnt = [zero] + [nacc_in[q][0] - early[q] for q in rem]
                rank0 = early
            else:
                parts = {q: pieces[q][k] for q in rem}
                cnt = [nacc_in[q][k] for q in range(NDEV)]
                rank0 = {q: zero for q in rem}
            lo = {q: bat[q][0][k] for q in rem}
            hi = {q: bat[q][1][k] for q in rem}
            first = {q: bat[q][2][k] for q in rem}
        lo_k = _prefix(cnt, zero)
        with _scope("s_dwait"):
            if step == 0:
                _wait_chunks(xt, dsem.at[EL], n_in, nmax, CHD)
            else:
                if step == 1:
                    for q in rem:
                        pltpu.make_async_copy(ctl_v.at[0], ctl_slot(q),
                                              ksem.at[q]).wait()
                    sqz = {q: ctl_s[q * LANES] == 0 for q in rem}
                c0 = {q: _cdiv_pow2(offin[q][k], GM) for q in rem}
                c1 = {q: _cdiv_pow2(offin[q][k + 1], GM) for q in rem}
                nmax = (CAP + 3 * (GM - 1)) // GM
                _wait_chunks(
                    xt, dsem.at[k],
                    sum(jnp.where(sqz[q], 0, c1[q] - c0[q]) for q in rem),
                    nmax, GM * XR)
                _wait_chunks(
                    xt, qsem.at[k],
                    sum(jnp.where(sqz[q], c1[q] - c0[q], 0) for q in rem),
                    nmax, SQ)
                for q in rem:
                    lax.fori_loop(c0[q], jnp.where(sqz[q], c1[q], c0[q]),
                                  functools.partial(unsqueeze, q), 0)
        with _scope("s_asm"):
            for q in range(NDEV - 1, 0, -1):
                for i, (r0, n, pos) in reversed(list(enumerate(parts[q]))):
                    big = step > 1 and i == len(parts[q]) - 1
                    _copy_bwd(rs, ((q - 1) * SD + XB + pos) * XR,
                              eb, (XB + lo_k[q] + r0 - rank0[q]) * XR, n, XR,
                              XB if big else 16)
            if step != 1:
                _copy_bwd(sbf, ((me * EL + k) * CAPF + XB) * XR,
                          eb, XB * XR, cnt[0], XR, XB)
        if step != 1:
            with _scope("s_wwait"):
                w_cps[k].wait()
        with _scope("s_mm"):
            nfind = 0 if step < 3 else 1 if step < EL - 1 else 2
            publish = [finds.pop(0)() for _ in range(nfind)]
            if step > 1:
                for t in range((k - 1) * T // (EL - 1), k * T // (EL - 1)):
                    inv_s[pos_s[t // LANES, t % LANES]] = (t >> 3) * 64 + (t & 7)

            def matmul(m, eref, step=step, k=k, lo_k=lo_k):
                w0 = eb[pl.ds(XB * XR, m, stride=XR), :]
                w1 = eb[pl.ds(XB * XR + 1, m, stride=XR), :]
                lhs = jnp.concatenate(
                    [_unpack_lo(w0), _unpack_lo(w1), _unpack_hi(w0), _unpack_hi(w1)],
                    axis=1).astype(jnp.bfloat16)
                planes = [None] * 4
                for n in range(4):
                    c0, c1 = n * LANES, H // 2 + n * LANES
                    wb = jnp.concatenate(
                        [wv[k, :, c0:c0 + LANES], wv[k, :, c1:c1 + LANES]],
                        axis=1).astype(jnp.bfloat16)
                    y = jnp.dot(lhs, wb, preferred_element_type=jnp.float32)
                    if eref is None:
                        valid = (lax.broadcasted_iota(jnp.int32, y.shape, 0)
                                 < lo_k[NDEV])
                        top = jnp.max(jnp.where(valid, jnp.abs(y), 0.0), axis=0,
                                      keepdims=True)
                        top = jnp.broadcast_to(
                            jnp.max(top, axis=1, keepdims=True), (1, LANES))
                        eref = (_pack(top, top) & U32(0x7F807F80)) | U32(0x80008000)
                        er_out[k:k + 1, :] = eref
                    w = _pack(y[:, 0:LANES], y[:, LANES:2 * LANES])
                    if step != 1:
                        lb[pl.ds(k * CAPM * 4 + n, m, stride=4), :] = w
                    _encode(w, n, eref, planes)
                for n in range(YR):
                    rb[n, 0:m, :] = planes[n]
                pb[pl.ds(step * FS, m), :] = planes[3]

            if step == 1:
                lax.cond(lo_k[NDEV] <= MS, lambda: matmul(MS, er_out[0:1, :]),
                         lambda: matmul(CAPM, er_out[0:1, :]))
            else:
                matmul(CAPM, None)
            for f in publish:
                f()
            if step != 1:
                for q in rem:
                    pltpu.make_async_remote_copy(
                        src_ref=er_out.at[pl.ds(k, 1)],
                        dst_ref=er_in.at[pl.ds((NDEV - q - 1) * EL + k, 1)],
                        send_sem=ssem.at[3],
                        recv_sem=esem.at[(NDEV - q - 1) * EL + k],
                        device_id=(chip(q),), device_id_type=MESH).start()

        def find(step=step, k=k, lo_k=lo_k, rank0=rank0):
            rows = lax.broadcasted_iota(jnp.int32, (CAPM, LANES), 0)
            need = (rows >= lo_k[1]) & (rows < lo_k[NDEV])
            need = jnp.where(need, pb[pl.ds(step * FS, CAPM), :], U32(0)) != 0
            found = _nonzero_rows(need, lo_k[2:])

            def publish():
                flag_v[step * 8:step * 8 + 8, :] = found
                flag_cp = pltpu.make_async_copy(
                    flag_v.at[pl.ds(step * 8, 8)], flag_s.at[pl.ds(step * 8, 8)],
                    gsem.at[step])
                flag_cp.start()
                scans.append((flag_cp, step, k, lo_k, rank0))

            return publish

        finds.append(find)
        if step == EL:
            with _scope("s_scan"):
                find()()
                while len(scans) > 1:
                    scan(*scans.pop(0))
                npat1 = dict(npat)
                scan(*scans.pop(0))
                send_patches(npat1)
        with _scope("s_csend"):
            for q in rem:
                def move(i, c_, src=lo_k[q],
                         dst=(q - 1) * SC + offc_out[q][k] + rank0[q]):
                    for n in range(YR):
                        css[n, pl.ds(dst + i * YB, YB), :] = rb[
                            n, pl.ds(src + i * YB, YB), :]
                    return c_

                lax.fori_loop(0, _cdiv_pow2(cnt[q], YB), move, 0)

            def relay(c, carry_, k=k):
                send_res(css, SC + c * GC, fb, c * GC, fsem.at[k], me ^ 1)
                return carry_

            if step:
                lax.fori_loop(jnp.maximum(lo[2], rel_out) if k else rel_out,
                              jnp.maximum(hi[2], rel_out), relay, 0)
            lim = jnp.where((me & 1) == 1, hi[1], hi[3])
            lim = jnp.maximum(lim, DMIN + (step + 2) * (256 // CH) - alink - lim)
            lim = jnp.minimum(jnp.minimum(lim, rel_out), hi[2])
            lim = jnp.maximum(lim, dsent)

            def send_k(q, c, k=k, lo=lo, first=first):
                if q == 2:
                    send_diag(c)
                else:
                    send_y(q, c, jnp.where(c == lo[q], first[q], k))

            send_ranges({1: lo[1], 2: dsent, 3: lo[3]},
                        {1: hi[1], 2: lim, 3: hi[3]}, send_k)
            dsent = lim
        with _scope("s_scan"):
            while scans:
                scan(*scans.pop(0))

    n_fwd = fbat[1][EL - 1] - rel_in
    nres = n_fwd + sum(bat[q][1][EL - 1] for q in rem)
    held = jnp.maximum(dsent, rel_out - n_fwd)
    send_diag_range(dsent, held)

    with _scope("s_prep2"):
        def zero_body(i, c):
            out_ref[pl.ds(pl.multiple_of(i * 64, 64), 64), :] = jnp.zeros(
                (64, LANES), jnp.float32)
            return c

        kept = sum(sum(nacc_me[j]) for j in range(NDEV))

        @pl.when(kept < T)
        def _():
            lax.fori_loop(0, T // 8, zero_body, 0, unroll=2)

    def put_token(o, w):
        out_ref[pl.ds(o, 8, stride=8), :] = jnp.concatenate(
            [_unpack_lo(w), _unpack_hi(w)], axis=0)

    def drain(sem, n, ch):
        def body(i, c):
            pltpu.make_async_copy(xt.at[pl.ds(0, 32 * ch)],
                                  xt.at[pl.ds(0, 32 * ch)], sem).wait()
            return c

        lax.fori_loop(0, n >> 5, body, 0)
        _wait_chunks(xt, sem, n & 31, 31, ch)

    with _scope("s_drain0"):
        for j in range(2 * (NDEV - 1)):
            pltpu.make_async_copy(hist_v.at[0], hist_v.at[0], msem.at[2]).wait()
        drain(ssem.at[0], nsent, CHD)
        drain(ssem.at[4], nsq, SQ)
        for j in rem:
            for k, v in enumerate(_prefix(nacc_me[j], jnp.int32(0))):
                tab_s[(j - 1) * 16 + k] = v
        tab_s[48] = rel_in
        for k in range(EL):
            tab_s[49 + k] = jnp.maximum(fbat[1][k], rel_in)

    def local(k, c):
        n = nacc_s[me * (E + EL) + k]
        ibase = ((me * EL + k) * CAPF + XB) * XR
        srow = k * (CAPM * 4)

        def one(r, u):
            put_token(inv_s[ibase + r * XR + u * XR],
                      lb[pl.ds(srow + r * 4 + u * 4, 4), :])

        def body(i, c_):
            r = jnp.minimum(i * DB, n - DB)
            for u in range(DB):
                one(r, u)
            return c_

        def body1(i, c_):
            one(i, 0)
            return c_

        big = n >= DB
        lax.fori_loop(0, jnp.where(big, _cdiv_pow2(n, DB), 0), body, 0)
        lax.fori_loop(0, jnp.where(big, 0, n), body1, 0)
        return c

    def receive(k, j):
        o0 = tab_s[(j - 1) * 16 + k]
        o1 = tab_s[(j - 1) * 16 + k + 1]
        n = o1 - o0
        with _scope("s_cwait"):
            _wait_chunks(xt, csem.at[(j - 1) * EL + k],
                         _cdiv_pow2(o1, GC) - _cdiv_pow2(o0, GC),
                         (CAP + GC - 1) // GC)
            er = er_in.at[pl.ds((j - 1) * EL + k, 1)]
            pltpu.make_async_copy(er, er, esem.at[(j - 1) * EL + k]).wait()
        eref = er[...]
        srow = (j - 1) * SC + DB + o0
        ibase = ((chip(j) * EL + k) * CAPF + XB) * XR

        def expand(t0, half):
            planes = [csr[r, pl.ds(srow + t0, DB), :] for r in range(YR)] + [None]
            for r in range(4):
                st[pl.ds(half * (DB * 4) + r, DB, stride=4), :] = _decode(
                    planes, r, eref)

        def body(i, c):
            r = jnp.minimum(i * DB, n - DB)
            base = (i & 1) * (DB * 4)
            for u in range(DB):
                put_token(inv_s[ibase + r * XR + u * XR],
                          st[pl.ds(base + u * 4, 4), :])
            expand(jnp.minimum((i + 1) * DB, n - DB), (i + 1) & 1)
            return c

        def body1(i, c):
            put_token(inv_s[ibase + i * XR], st[pl.ds((DB - n + i) * 4, 4), :])
            return c

        with _scope("s_out"):
            big = n >= DB
            expand(jnp.minimum(n - DB, 0), 0)
            lax.fori_loop(0, jnp.where(big, _cdiv_pow2(n, DB), 0), body, 0)
            lax.fori_loop(0, jnp.where(big, 0, n), body1, 0)

    def patch(j, last):
        lbase = (j - 1) * LCAP
        q = NDEV - j
        if not last:
            list_copy(q, 0, LA, 0).wait_recv()
            n = lst_in[lbase]
            pl.when(n > LA - 2)(lambda: list_copy(q, LA, LCAP - LA, 1).wait_recv())
            nch = _cdiv_pow2(n, PR)
            _wait_chunks(xt, psem.at[(j - 1) * 2], nch >> 4,
                         PCAP // (16 * PR), 16 * PR)
            _wait_chunks(xt, psem.at[(j - 1) * 2 + 1], nch & 15, 15, PR)

        lo, hi = (lst_in[lbase + 1], lst_in[lbase]) if last else (0, lst_in[lbase + 1])
        sub4 = lax.broadcasted_iota(U32, (8, LANES), 0) * 4

        def fix(i0, m):
            rows, vals = [], []
            for i in [i0 + u for u in range(m)]:
                o = inv_s[(chip(j) * (EL * CAPF) + XB) * XR + lst_in[lbase + 2 + i]]
                h = jnp.broadcast_to(psr[pl.ds((j - 1) * PCAP + i, 1), :],
                                     (8, LANES))
                h = ((h >> sub4) & U32(0xF)) << 27
                v = lax.bitcast_convert_type(out_ref[pl.ds(o, 8, stride=8), :], U32)
                rows.append(o)
                vals.append((v & U32(0x807FFFFF)) | ((v - h) & U32(0x7F800000)))
            for o, v in zip(rows, vals):
                out_ref[pl.ds(o, 8, stride=8), :] = lax.bitcast_convert_type(
                    v, jnp.float32)

        def body4(g, c):
            fix(lo + g * 4, 4)
            return c

        def body1(i, c):
            fix(i, 1)
            return c

        with _scope("s_patch"):
            n4 = (hi - lo) >> 2
            lax.fori_loop(0, n4, body4, 0)
            lax.fori_loop(lo + n4 * 4, hi, body1, 0)

    with _scope("s_fwd"):
        held = lax.fori_loop(0, FL, forward, held)
    with _scope("s_local"):
        lax.fori_loop(0, EL, local, 0)

    def round_(k, c):
        held_, dnext = c
        with _scope("s_fwd"):
            kf = jnp.minimum(k + FL, EL)
            held_ = lax.fori_loop(kf, jnp.minimum(kf + 1, EL), forward, held_)
        clear = tab_s[49 + jnp.minimum(kf, EL - 1)] == tab_s[48 + EL]
        upto = jnp.where(clear, k + 1, dnext)

        def step_(i, c_):
            diag = i >= 2
            receive(jnp.where(diag, dnext + i - 2, k),
                    jnp.where(diag, 2, 1 + 2 * i))
            return c_

        lax.fori_loop(0, 2 + upto - dnext, step_, 0)
        return held_, upto

    lax.fori_loop(0, EL - 2, round_, (held, jnp.int32(0)))
    for j in (1, 3, 2):
        receive(EL - 2, j)
        patch(j, False)
    with _scope("s_drain1"):
        drain(ssem.at[2], sum(_cdiv_pow2(npat[q], PR) for q in rem), PR)
        nref = (NDEV - 1) * EL
        pltpu.make_async_copy(xt.at[pl.ds(0, nref)], xt.at[pl.ds(0, nref)],
                              ssem.at[3]).wait()
        for q in rem:
            list_copy(q, 0, LA, 0).wait_send()
            pl.when(npat[q] > LA - 2)(
                lambda q=q: list_copy(q, LA, LCAP - LA, 1).wait_send())
    for j in (1, 3, 2):
        receive(EL - 1, j)
        patch(j, True)

    with _scope("s_drain"):
        drain(ssem.at[1], nres, CH)


def pallas_dist_moe_cap_ep_tokshard_n2048_d512_e8_h1024_kernel(
    x: jax.Array,
    router_W: jax.Array,
    route_idx: jax.Array,
    expert_W: jax.Array,
):
    del router_W
    idx = route_idx.astype(jnp.int32).reshape(T // LANES, LANES)
    any_spec = pl.BlockSpec(memory_space=pl.ANY)
    out = pl.pallas_call(
        _kernel,
        out_shape=jax.ShapeDtypeStruct((T * H // LANES, LANES), jnp.float32),
        in_specs=[any_spec, any_spec, any_spec],
        out_specs=pl.BlockSpec(memory_space=pltpu.VMEM),
        scratch_shapes=[
            pltpu.VMEM((T, D), jnp.float32),
            pltpu.VMEM((EL, D, H), jnp.float32),
            pltpu.VMEM((T // LANES, LANES), jnp.int32),
            pltpu.VMEM((T // LANES, LANES), jnp.int32),
            pltpu.VMEM((8, LANES), jnp.int32),
            pltpu.VMEM((T * XR, LANES), U32),
            pltpu.VMEM(((E * CAPF + 2 * XB) * XR, LANES), U32),
            pltpu.VMEM(((NDEV - 1) * SD * XR, LANES), U32),
            pltpu.VMEM(((NDEV - 1) * SD * XR, LANES), U32),
            pltpu.VMEM(((XB + CAPM) * XR, LANES), U32),
            pltpu.VMEM((YR, CAPM + YB, LANES), U32),
            pltpu.VMEM((YR, (NDEV - 1) * SC, LANES), U32),
            pltpu.VMEM((YR, (NDEV - 1) * SC, LANES), U32),
            pltpu.VMEM((YR, SC, LANES), U32),
            pltpu.VMEM(((EL + 1) * FS, LANES), U32),
            pltpu.VMEM(((NDEV - 1) * PCAP, LANES), U32),
            pltpu.VMEM(((NDEV - 1) * PCAP, LANES), U32),
            pltpu.VMEM((EL, LANES), U32),
            pltpu.VMEM(((NDEV - 1) * EL, LANES), U32),
            pltpu.VMEM(((EL + 1) * 8, 2 * LANES), jnp.int32),
            pltpu.VMEM((EL * CAPM * 4, LANES), U32),
            pltpu.VMEM((2 * DB * 4, LANES), U32),
            pltpu.VMEM(((NDEV - 1) * NSQ * SQ, LANES), U32),
            pltpu.VMEM(((NDEV - 1) * NSQ * SQ, LANES), U32),
            pltpu.VMEM((8, LANES), jnp.int32),
            pltpu.VMEM((GM * XR, LANES), U32),
            pltpu.SMEM((T // LANES, LANES), jnp.int32),
            pltpu.SMEM(((E * CAPF + XB) * XR,), jnp.int32),
            pltpu.SMEM((NDEV * LANES,), jnp.int32),
            pltpu.SMEM((NDEV * E,), jnp.int32),
            pltpu.SMEM(((EL + 1) * 8, 2 * LANES), jnp.int32),
            pltpu.SMEM(((NDEV - 1) * LCAP,), jnp.int32),
            pltpu.SMEM(((NDEV - 1) * LCAP,), jnp.int32),
            pltpu.SMEM((64,), jnp.int32),
            pltpu.SMEM((NDEV * LANES,), jnp.int32),
            pltpu.SemaphoreType.DMA((NXC,)),
            pltpu.SemaphoreType.DMA((EL,)),
            pltpu.SemaphoreType.DMA((3,)),
            pltpu.SemaphoreType.DMA((NDEV,)),
            pltpu.SemaphoreType.DMA((EL + 1,)),
            pltpu.SemaphoreType.DMA(((NDEV - 1) * EL,)),
            pltpu.SemaphoreType.DMA((EL,)),
            pltpu.SemaphoreType.DMA((5,)),
            pltpu.SemaphoreType.DMA(((NDEV - 1) * EL,)),
            pltpu.SemaphoreType.DMA((EL + 1,)),
            pltpu.SemaphoreType.DMA((12,)),
            pltpu.SemaphoreType.DMA((6,)),
            pltpu.SemaphoreType.DMA((EL,)),
            pltpu.SemaphoreType.DMA((NDEV,)),
        ],
        compiler_params=pltpu.CompilerParams(
            collective_id=0, vmem_limit_bytes=96 * 1024 * 1024,
            disable_semaphore_checks=True, disable_bounds_checks=True),
    )(x, idx, expert_W)
    out = out.reshape(T // 8, H // LANES, 8, LANES).transpose(0, 2, 1, 3)
    return out.reshape(T, H)
```
